```python
import numpy as np

kernel_name = "dist_mean_ax0_xy_m1024_n512"

def setup_inputs():
    return {"x": np.random.randn(2048, 1024).astype(np.float32)}

def reference(x: np.ndarray) -> np.ndarray:
    return np.mean(x, axis=0, keepdims=True)
```

```python
import jax
import jax.numpy as jnp
from jax import lax
from jax.experimental import pallas as pl
from jax.experimental.pallas import tpu as pltpu


def pallas_dist_mean_ax0_xy_m1024_n512_kernel(x: jax.Array):
    m, n = x.shape
    inv = 1.0 / (m * 2)

    def body(x_ref, o_ref, send_buf, recv_buf, send_sem, recv_sem):
        my_x = lax.axis_index("x")
        my_y = lax.axis_index("y")
        peer = (1 - my_x, my_y)
        bar = pltpu.get_barrier_semaphore()
        pl.semaphore_signal(bar, inc=1, device_id=peer,
                            device_id_type=pl.DeviceIdType.MESH)
        part = jnp.sum(x_ref[...], axis=0, keepdims=True)
        send_buf[...] = part
        pl.semaphore_wait(bar, 1)
        rdma = pltpu.make_async_remote_copy(
            src_ref=send_buf, dst_ref=recv_buf, send_sem=send_sem,
            recv_sem=recv_sem, device_id=peer,
            device_id_type=pl.DeviceIdType.MESH)
        rdma.start()
        rdma.wait()
        o_ref[...] = (part + recv_buf[...]) * inv

    return pl.pallas_call(
        body,
        out_shape=jax.ShapeDtypeStruct((1, n), x.dtype),
        in_specs=[pl.BlockSpec(memory_space=pltpu.VMEM)],
        out_specs=pl.BlockSpec(memory_space=pltpu.VMEM),
        scratch_shapes=[
            pltpu.VMEM((1, n), jnp.float32),
            pltpu.VMEM((1, n), jnp.float32),
            pltpu.SemaphoreType.DMA,
            pltpu.SemaphoreType.DMA,
        ],
        compiler_params=pltpu.CompilerParams(collective_id=0),
    )(x)
```

```python
import jax
import jax.numpy as jnp
from jax import lax
from jax.experimental import pallas as pl
from jax.experimental.pallas import tpu as pltpu

_X_SIZE = 2
_SUBLANES = 8


def _row_chunks(m):
    last = 2 * _SUBLANES
    mid = m // 4 - last
    return (m - mid - last, mid, last)


def pallas_dist_mean_ax0_xy_m1024_n512_kernel(
    x: jax.Array,
):
    m, n = x.shape
    assert m % (4 * _SUBLANES) == 0 and m // 4 > 2 * _SUBLANES
    inv_rows = 1.0 / (m * _X_SIZE)
    sizes = _row_chunks(m)
    offs = tuple(sum(sizes[:c]) for c in range(len(sizes)))

    def body(x_hbm, o_ref, x_vmem, send_buf, recv_buf, in_sems, send_sem, recv_sem):
        copies = [
            pltpu.make_async_copy(
                x_hbm.at[pl.ds(off, size)],
                x_vmem.at[pl.ds(off, size)],
                in_sems.at[c],
            )
            for c, (off, size) in enumerate(zip(offs, sizes))
        ]
        for cp in copies:
            cp.start()

        peer = (1 - lax.axis_index("x"), lax.axis_index("y"))
        barrier = pltpu.get_barrier_semaphore()
        pl.semaphore_signal(
            barrier, inc=1, device_id=peer, device_id_type=pl.DeviceIdType.MESH
        )

        acc = None
        for c, (off, size) in enumerate(zip(offs, sizes)):
            copies[c].wait()
            for r in range(off, off + size, _SUBLANES):
                rows = x_vmem[pl.ds(r, _SUBLANES), :]
                acc = rows if acc is None else acc + rows
            if c == len(sizes) - 2:
                pl.semaphore_wait(barrier, 1)

        send_buf[...] = jnp.sum(acc, axis=0, keepdims=True) * inv_rows
        rdma = pltpu.make_async_remote_copy(
            src_ref=send_buf,
            dst_ref=recv_buf,
            send_sem=send_sem,
            recv_sem=recv_sem,
            device_id=peer,
            device_id_type=pl.DeviceIdType.MESH,
        )
        rdma.start()
        rdma.wait_recv()
        o_ref[...] = send_buf[...] + recv_buf[...]
        rdma.wait_send()

    return pl.pallas_call(
        body,
        out_shape=pltpu.VMEM((1, n), x.dtype),
        in_specs=[pl.BlockSpec(memory_space=pl.ANY)],
        out_specs=pl.BlockSpec(memory_space=pltpu.VMEM),
        scratch_shapes=[
            pltpu.VMEM((m, n), x.dtype),
            pltpu.VMEM((1, n), x.dtype),
            pltpu.VMEM((1, n), x.dtype),
            pltpu.SemaphoreType.DMA((len(sizes),)),
            pltpu.SemaphoreType.DMA,
            pltpu.SemaphoreType.DMA,
        ],
        compiler_params=pltpu.CompilerParams(
            collective_id=0,
            disable_bounds_checks=True,
            disable_semaphore_checks=True,
        ),
    )(x)
```
